```python
import numpy as np

kernel_name = "dist_rmsnorm_colshard_i_m768_n512"

def setup_inputs():
    x = np.random.randn(768, 2048).astype(np.float32)
    gamma = np.random.randn(2048).astype(np.float32)
    return {"x": x, "gamma": gamma}

def reference(x: np.ndarray, gamma: np.ndarray) -> np.ndarray:
    eps = 1e-5
    rms = np.sqrt(np.mean(x * x, axis=1, keepdims=True) + eps)
    return gamma * x / rms
```

```python
import numpy as np
import jax, jax.numpy as jnp
from jax import lax
from jax.experimental import pallas as pl
from jax.experimental.pallas import tpu as pltpu
M, N, ND = 768, 512, 4
HBM = pltpu.MemorySpace.HBM
MESH = pl.DeviceIdType.MESH

def make(groups=(((128, 128), (128, 128), (128,)), ((128,),)), prio=0, nochecks=True, flags=None, order=(2, 1, 3), split_last=True):
    G, r, p, plan = len(groups), 0, 0, []
    for grp in groups:
        lds = []
        for ld in grp:
            pcs = []
            for n in ld:
                pcs.append((p, r, n)); p += 1; r += n
            lds.append(pcs)
        plan.append(lds)
    assert r == M
    NP, NL = p, sum(len(g) for g in groups)
    def body(x_hbm, g_hbm, o_ref, xv, gv, part, ld_sem, g_sem, s_sem, r_sem):
        loads = []
        for lds in plan:
            for pcs in lds:
                rows = pl.ds(pcs[0][1], sum(q[2] for q in pcs))
                loads.append(pltpu.make_async_copy(x_hbm.at[rows], xv.at[rows], ld_sem.at[len(loads)]))
        loads[0].start(priority=prio)
        me = lax.axis_index("i")
        peer = {k: (me + k) % ND for k in order}
        bar = pltpu.get_barrier_semaphore()
        for k in order:
            pl.semaphore_signal(bar, inc=1, device_id=(peer[k],), device_id_type=MESH)
        for d in loads[1:]: d.start(priority=prio)
        gcp = pltpu.make_async_copy(g_hbm, gv, g_sem)
        gcp.start(priority=prio)
        def rdma(g, k):
            sl = pl.ds(plan[g][0][0][0], sum(len(pcs) for pcs in plan[g]))
            return pltpu.make_async_remote_copy(part.at[0, sl], part.at[k, sl], s_sem.at[g * 3 + k - 1], r_sem.at[g * 3 + k - 1],
                device_id=(peer[k],), device_id_type=MESH)
        def eye(n):
            return lax.broadcasted_iota(jnp.int32, (n, 128), 0) == lax.broadcasted_iota(jnp.int32, (n, 128), 1)
        i = 0
        for g, lds in enumerate(plan):
            for pcs in lds:
                loads[i].wait(); i += 1
                for p, r0, n in pcs:
                    t = [xv[pl.ds(r0, n), pl.ds(j * 128, 128)] for j in range(4)]
                    s = jnp.sum((t[0] * t[0] + t[1] * t[1]) + (t[2] * t[2] + t[3] * t[3]), axis=1, keepdims=True)
                    part[0, p] = jnp.sum(jnp.where(eye(n), s, 0.0), axis=0, keepdims=True)
            if g == 0:
                pl.semaphore_wait(bar, 3)
            for k in order: rdma(g, k).start()
        gcp.wait()
        gv[...] = gv[...] * np.float32(np.sqrt(N * ND))
        for g, lds in enumerate(plan):
            pcs = [q for l in lds for q in l]
            if g == G - 1:
                for gg in range(G):
                    for k in order: rdma(gg, k).wait_send()
            for k in (1, 3): rdma(g, k).wait_recv()
            if not split_last: rdma(g, 2).wait_recv()
            pre = [(part[0, p] + np.float32(1e-5 * N * ND)) + (part[1, p] + part[3, p]) for p, _, _ in pcs]
            if split_last: rdma(g, 2).wait_recv()
            for (p, r0, n), a in zip(pcs, pre):
                rt = jnp.sum(jnp.where(eye(n), lax.rsqrt(a + part[2, p]), 0.0), axis=1, keepdims=True)
                for j in range(4):
                    cols = pl.ds(j * 128, 128)
                    o_ref[pl.ds(r0, n), cols] = xv[pl.ds(r0, n), cols] * gv[:, cols] * rt
    def f(x, g):
        return pl.pallas_call(body, out_shape=pltpu.VMEM((M, N), jnp.float32),
            in_specs=[pl.BlockSpec(memory_space=HBM)] * 2, out_specs=pl.BlockSpec(memory_space=pltpu.VMEM),
            scratch_shapes=[pltpu.VMEM((M, N), jnp.float32), pltpu.VMEM((1, N), jnp.float32), pltpu.VMEM((ND, NP, 1, 128), jnp.float32),
                pltpu.SemaphoreType.DMA((NL,)), pltpu.SemaphoreType.DMA, pltpu.SemaphoreType.DMA((3 * G,)), pltpu.SemaphoreType.DMA((3 * G,))],
            compiler_params=pltpu.CompilerParams(collective_id=0, disable_bounds_checks=nochecks, disable_semaphore_checks=nochecks, flags=flags))(x, g.reshape(1, N))
    return f
_PLAN = (((128, 128), (128, 128)), ((128,), (64,)), ((64,),))


def pallas_dist_rmsnorm_colshard_i_m768_n512_kernel(x, gamma):
    return make(_PLAN)(x, gamma)
```

```python
import jax
import jax.numpy as jnp
from jax import lax
from jax.experimental import pallas as pl
from jax.experimental.pallas import tpu as pltpu

N_DEV = 4
EPS = 1e-5
SUBLANES, LANES = 8, 128

BULK_BLOCKS = (128, 128, 128, 128, 128)
TAIL_BLOCKS = (80, 48)
FIRST_SEND = 3

OWN, FAR, NEAR = 0, 2, (1, 3)

_SIZES = BULK_BLOCKS + TAIL_BLOCKS
_BLOCKS = tuple((sum(_SIZES[:b]), n) for b, n in enumerate(_SIZES))
_N_BULK = len(BULK_BLOCKS)
_TAIL_ROW = sum(BULK_BLOCKS)
_N_MSGS = len(_BLOCKS) - FIRST_SEND + 1 + len(NEAR)


def _iota(rows, dim):
    return lax.broadcasted_iota(jnp.int32, (rows, LANES), dim)


def _column_to_lanes(col):
    acc = jnp.zeros((SUBLANES, LANES), col.dtype)
    for i in range(0, col.shape[0], SUBLANES):
        here = _iota(SUBLANES, 1) == _iota(SUBLANES, 0) + i
        acc = jnp.where(here, col[i : i + SUBLANES], acc)
    return jnp.sum(acc, axis=0, keepdims=True)


def _lanes_to_column(row, n):
    diag = jnp.where(_iota(n, 0) == _iota(n, 1), row, 0.0)
    return jnp.sum(diag, axis=1, keepdims=True)


def _scalars_to_rows(scalars):
    rows = [jnp.full((SUBLANES, LANES), s, s.dtype) for s in scalars]
    for bit in (1, 2, 4):
        low = (_iota(SUBLANES, 0) & bit) == 0
        rows = [jnp.where(low, a, b) for a, b in zip(rows[::2], rows[1::2])]
    return rows[0]


def _body(
    x_hbm,
    gamma_hbm,
    out_ref,
    x_ref,
    gamma_ref,
    sums_ref,
    far_tail_ref,
    tail_ref,
    load_sems,
    send_sems,
    recv_sems,
):
    n_cols = x_ref.shape[1]
    col_tiles = [pl.ds(c, LANES) for c in range(0, n_cols, LANES)]

    x_loads = [
        pltpu.make_async_copy(
            x_hbm.at[pl.ds(r, n)], x_ref.at[pl.ds(r, n)], load_sems.at[b]
        )
        for b, (r, n) in enumerate(_BLOCKS)
    ]
    gamma_load = pltpu.make_async_copy(
        gamma_hbm, gamma_ref, load_sems.at[len(_BLOCKS)]
    )

    x_loads[0].start()
    me = lax.axis_index("i")
    peers = {k: (me + k) % N_DEV for k in (FAR, *NEAR)}
    barrier = pltpu.get_barrier_semaphore()
    for peer in peers.values():
        pl.semaphore_signal(
            barrier, inc=1, device_id=(peer,), device_id_type=pl.DeviceIdType.MESH
        )
    for load in x_loads[1:]:
        load.start()
    gamma_load.start()

    sent = []

    def send(src, dst, k):
        copy = pltpu.make_async_remote_copy(
            src_ref=src,
            dst_ref=dst,
            send_sem=send_sems.at[len(sent)],
            recv_sem=recv_sems.at[len(sent)],
            device_id=(peers[k],),
            device_id_type=pl.DeviceIdType.MESH,
        )
        copy.start()
        sent.append(copy)
        return copy

    far = {}
    for b, (r, n) in enumerate(_BLOCKS):
        x_loads[b].wait()
        squares = [jnp.square(x_ref[pl.ds(r, n), cols]) for cols in col_tiles]
        while len(squares) > 1:
            squares = [p + q for p, q in zip(squares[::2], squares[1::2], strict=True)]
        sums_ref[OWN, b] = _column_to_lanes(jnp.sum(squares[0], axis=1, keepdims=True))

        if b == FIRST_SEND - 1:
            pl.semaphore_wait(barrier, N_DEV - 1)
            head = pl.ds(0, FIRST_SEND)
            far[0] = send(sums_ref.at[OWN, head], sums_ref.at[FAR, head], FAR)
        elif b >= _N_BULK:
            far[b] = send(sums_ref.at[OWN, b], far_tail_ref.at[b - _N_BULK], FAR)
        elif b >= FIRST_SEND:
            far[b] = send(sums_ref.at[OWN, b], sums_ref.at[FAR, b], FAR)
    near = [send(sums_ref.at[OWN], sums_ref.at[k], k) for k in NEAR]

    def all_but_far(b):
        return sums_ref[OWN, b] + (sums_ref[NEAR[0], b] + sums_ref[NEAR[1], b])

    def inv_rms(total):
        return lax.rsqrt(total * (1.0 / (n_cols * N_DEV)) + EPS)

    def write(rows, scale):
        for cols in col_tiles:
            out_ref[rows, cols] = gamma_ref[:, cols] * x_ref[rows, cols] * scale

    gamma_load.wait()
    for copy in near:
        copy.wait_recv()
    for b in range(_N_BULK, len(_BLOCKS)):
        r, n = _BLOCKS[b]
        tail_ref[pl.ds(r - _TAIL_ROW, n), :] = jnp.broadcast_to(
            _lanes_to_column(all_but_far(b), n), (n, LANES)
        )

    for b, (r, n) in enumerate(_BLOCKS):
        if b == len(_BLOCKS) - 1:
            for copy in sent:
                copy.wait_send()
        if b in far:
            far[b].wait_recv()
        if b < _N_BULK:
            total = all_but_far(b) + sums_ref[FAR, b]
            write(pl.ds(r, n), _lanes_to_column(inv_rms(total), n))
        else:
            for i in range(0, n, SUBLANES):
                far_sums = _scalars_to_rows(
                    [far_tail_ref[b - _N_BULK, 0, i + j] for j in range(SUBLANES)]
                )
                total = tail_ref[pl.ds(r + i - _TAIL_ROW, SUBLANES), :] + far_sums
                write(pl.ds(r + i, SUBLANES), inv_rms(total))


def pallas_dist_rmsnorm_colshard_i_m768_n512_kernel(
    x: jax.Array,
    gamma: jax.Array,
):
    m, n = x.shape
    assert m == sum(_SIZES) and n % LANES == 0 and x.dtype == jnp.float32
    return pl.pallas_call(
        _body,
        out_shape=jax.ShapeDtypeStruct((m, n), jnp.float32),
        in_specs=[pl.BlockSpec(memory_space=pltpu.MemorySpace.HBM)] * 2,
        out_specs=pl.BlockSpec(memory_space=pltpu.MemorySpace.VMEM),
        scratch_shapes=[
            pltpu.VMEM((m, n), x.dtype),
            pltpu.VMEM((1, n), gamma.dtype),
            pltpu.VMEM((N_DEV, len(_BLOCKS), 1, LANES), jnp.float32),
            pltpu.SMEM((len(TAIL_BLOCKS), 1, LANES), jnp.float32),
            pltpu.VMEM((sum(TAIL_BLOCKS), LANES), jnp.float32),
            pltpu.SemaphoreType.DMA((len(_BLOCKS) + 1,)),
            pltpu.SemaphoreType.DMA((_N_MSGS,)),
            pltpu.SemaphoreType.DMA((_N_MSGS,)),
        ],
        compiler_params=pltpu.CompilerParams(
            collective_id=0,
            disable_bounds_checks=True,
            disable_semaphore_checks=True,
        ),
    )(x, gamma.reshape(1, n))
```
